```python
import numpy as np

kernel_name = "dist_sparse_attn_strided_qseq_b1_sq1024_skv1024_hq8_dh128"

def setup_inputs():
    x = np.random.randn(1, 4096, 1024).astype(np.float32)
    Wq = np.random.randn(1024, 4096).astype(np.float32) * 0.02
    K_ext = np.random.randn(1, 1024, 32, 128).astype(np.float32)
    V_ext = np.random.randn(1, 1024, 32, 128).astype(np.float32)
    Wo = np.random.randn(4096, 1024).astype(np.float32) * 0.02
    return {"x": x, "Wq": Wq, "K_ext": K_ext, "V_ext": V_ext, "Wo": Wo}

def reference(x, Wq, K_ext, V_ext, Wo):
    B, Sq, Skv, Hq, Dh = 1, 4096, 1024, 32, 128
    Q = (x @ Wq).reshape(B, Sq, Hq, Dh)
    qb = (np.arange(Sq) // 64)[:, None]
    kb = (np.arange(Skv) // 64)[None, :]
    mask = (qb == kb) | ((kb % 4) == (qb % 4))
    scores = np.einsum('bihd,bjhd->bhij', Q, K_ext).astype(np.float32) * 0.08838834764831843
    scores = np.where(mask[None, None, :, :], scores, -1e9)
    scores_max = scores.max(axis=-1, keepdims=True)
    w = np.exp(scores - scores_max)
    row_keep = mask.any(axis=1)
    w_sum = np.where(row_keep[None, None, :, None], w.sum(axis=-1, keepdims=True), 1.0)
    w = w / w_sum
    w = np.where(row_keep[None, None, :, None], w, 0.0)
    ctx = np.einsum('bhij,bjhd->bihd', w, V_ext).reshape(B, Sq, Hq * Dh)
    return ctx @ Wo
```

```python
import jax
import jax.numpy as jnp
import numpy as np
from jax import lax
from jax.experimental import pallas as pl
from jax.experimental.pallas import tpu as pltpu

BF16, F32 = jnp.bfloat16, jnp.float32
Q_SCALE = 0.08838834764831843 * 1.4426950408889634
NT_DIMS = (((1,), (1,)), ((), ()))

L0, L1, L2, L3, R0, R1, R2, R3 = range(8)
SCHEDULE = (
    ("P", L0, 0), ("P", L1, 0), ("P", L2, 0), ("P", L3, 0), ("P", L0, 1),
    ("Q", L0, 0, L1, 1), ("Q", L1, 0, L2, 1), ("Q", L2, 0, L3, 1, L3, 0, R0, 0, R0, 0, R0, 1),
    ("A", L0, 1, L1, 1), ("A", L2, 1, L3, 1),
    ("Q", R0, 1, R1, 0, R1, 0, R1, 1), ("Q", R1, 1, R0, 2, R0, 2, R1, 2, R1, 2, L0, 2), ("Q", L0, 2, L1, 2, L1, 2, L2, 2, L2, 2, L3, 2),
    ("Q", L3, 2, R2, 0, R2, 0, R2, 1, R2, 1, R2, 2),
    ("Q", R2, 2, R0, 3, R0, 3, R1, 3, R1, 3, R2, 3), ("Q", R2, 3, R3, 0, R3, 0, R3, 1, R3, 1, R3, 2),
    ("O", 2, 1, 0), ("Q", R3, 2, R3, 3, R3, 3, L0, 3), ("O", 3, 1, 0), ("O", 2, 2, 1),
    ("Q", L0, 3, L1, 3, L1, 3, L2, 3, L2, 3, L3, 3), ("A", L3, 3), ("O", 2, 2, 2),
    ("O", 0, 2, 0), ("O", 0, 1, 1), ("O", 2, 1, 3), ("O", 3, 1, 3), ("O", 1, 1, 1), ("O", 0, 2, 2), ("O", 0, 2, 3))
LATE = ((1, 3),)
SPARE = 8
WQ_PIECES = ((0, 0, 64), (0, 64, 192), (0, 256, 128), (0, 384, 128), (1, 0, 384), (1, 384, 128))
X_PIECES = ((0, 0, 1), (0, 1, 3), (1, 0, 4), (2, 0, 4), (3, 0, 4))
QA_ORDER = "m5 k0 k2 m1 p0 k1 m7 p2 e0 k3 m4 p1 m2 p3 e1 m3 m6"
A_ORDER = "k0 k2 p0 p2 k1 k3 e0 p1 p3 e1"
P_ORDER = "m2 m5 m3 m4 m1 m7 m6"
O_ORDER = "m5 m2 m3 m7 m4 m1 m6"
LOADS = ((2, "kv_load", (0, 2)), (4, "kv_load", (0, 3)), (5, "kv_load", (1, 0)), (5, "kv_load", (1, 1)),
         (6, "kv_load", (1, 2)), (7, "kv_load", (1, 3)), (7, "kv_load", (2, None)), (8, "wo_load", None),
         (11, "kv_load", (3, None)),
         (13, "wo_ready", 0), (13, "wo_ready", 1), (13, "wo_ready", 2), (13, "wo_ready", 3))
UNITS = {"P": 2, "A": 2, "Q": 4}


def _body_of(step):
    return step[0], step[2] if step[0] == "O" else (len(step) - 1) // UNITS[step[0]]


BODIES = sorted({_body_of(step) for step in SCHEDULE})
TABLE_WIDTH = 2 + max(len(step) - 1 for step in SCHEDULE)


def _plan():
    events, rows, seen = {}, [], set()

    def before(step, *event):
        if event not in seen:
            seen.add(event)
            events.setdefault(step, []).append(event)

    for step, name, arg in LOADS:
        before(step, name, arg)
    for i, step in enumerate(SCHEDULE):
        kind, *arg = step
        body = BODIES.index(_body_of(step))
        if kind != "O":
            both = list(zip(arg[::2], arg[1::2]))
            attended, units = {"P": ([], both), "A": (both, []), "Q": (both[::2], both[1::2])}[kind]
            for slot, g in units:
                for p, piece in enumerate(X_PIECES):
                    if slot == 4 + piece[0]:
                        before(i, "x_recv", p)
                    elif slot == piece[0] > 0:
                        before(i, "x_ready", p)
                for p, piece in enumerate(WQ_PIECES):
                    if g == 2 + piece[0]:
                        before(i, "wq_recv", p)
                    elif g == piece[0] > 0:
                        before(i, "wq_ready", p)
            for slot, g in attended:
                before(i, "kv_wait", (g, slot % 4) if g < 2 else (g, None))
            rows.append((body, *arg))
        else:
            pair, _, c = arg
            blk = 2 * c + pair % 2
            before(i, "wo_recv", c)
            add = [blk + n if pair < 2 and (pair + n, c) not in LATE else SPARE for n in range(arg[1])]
            rows.append((body, pair, c, SPARE if pair < 2 else blk, *add))
    table = [(int(i in events), *row) + (0,) * (TABLE_WIDTH - 1 - len(row)) for i, row in enumerate(rows)]
    return np.asarray(table, np.int32).reshape(-1), events


def _dot(a, b):
    return jnp.dot(a, b, preferred_element_type=F32)


LHS = {1: (0, 1, 3), 2: (2, 1, 3), 3: (0,), 4: (3,), 5: (0, 1, 1), 6: (2, -1, 0), 7: (1, -1, 3)}
RHS = {1: (0, 1, 3), 2: (0,), 3: (1, -1, 3), 4: (2, -1, 0), 5: (3,), 6: (0, 1, 1), 7: (2, 1, 3)}
LHS_SUMS = [j for j in LHS if len(LHS[j]) > 1]
X_SUMS = 28
RHS_SUMS = [j for j in RHS if len(RHS[j]) > 1]


def _operand(spec, block):
    if len(spec) == 1:
        return block(spec[0]).astype(BF16)
    a, b = block(spec[0]).astype(F32), block(spec[2]).astype(F32)
    return (a + b if spec[1] > 0 else a - b).astype(BF16)


class _Strassen:
    USES = {1: ((0, 1), (3, 1)), 2: ((2, 1), (3, -1)), 3: ((1, 1), (3, 1)), 4: ((0, 1), (2, 1)),
            5: ((0, -1), (1, 1)), 6: ((3, 1),), 7: ((0, 1),)}

    def __init__(self, lhs, rhs, done):
        self.lhs, self.rhs, self.done = lhs, rhs, done
        self.acc = [None] * 4
        self.sign = [1] * 4
        self.missing = [4, 2, 2, 4]

    def product(self, j):
        m = _dot(self.lhs(j), self.rhs(j))
        for n, sign in self.USES[j]:
            if self.acc[n] is None:
                self.acc[n], self.sign[n] = m, sign
            elif self.sign[n] < 0:
                self.acc[n], self.sign[n] = m - self.acc[n], 1
            else:
                self.acc[n] = self.acc[n] + m if sign > 0 else self.acc[n] - m
            self.missing[n] -= 1
            if not self.missing[n]:
                self.done(n, self.acc[n])


def _body(tab, x_hbm, wq_hbm, k_hbm, v_hbm, wo_hbm, out_ref,
          xs, xb, wqs, wqb, wqc, wos, wob, kv, qs, lhs_ops, sendb, recvb,
          x_sem, wq_sem, wo_sem, kv_sem,
          send_sem, xr_sem, wqr_sem, wor_sem, pr_sem):
    me = lax.axis_index("i")
    row_peer = 3 - me
    head_peer = me ^ 1

    def remote(src, dst, ssem, rsem, peer):
        return pltpu.make_async_remote_copy(src, dst, ssem, rsem, device_id=(peer,),
                                            device_id_type=pl.DeviceIdType.MESH)

    def x_load(p):
        r, j0, n = X_PIECES[p]
        return pltpu.make_async_copy(x_hbm.at[pl.ds(j0, n), r], xs.at[r, pl.ds(j0, n)], x_sem.at[p])

    def x_send(p):
        r, j0, n = X_PIECES[p]
        rows = pl.ds(64 * j0, 64 * n)
        return remote(xb.at[r, rows], xb.at[4 + r, rows], send_sem.at[0], xr_sem.at[p], row_peer)

    def wq_load(p):
        g, r0, n = WQ_PIECES[p]
        return pltpu.make_async_copy(wq_hbm.at[:, pl.ds(r0, n), pl.ds(g * 512, 512)],
                                     wqs.at[g, :, pl.ds(r0, n)], wq_sem.at[p])

    def wq_send(p):
        g, r0, n = WQ_PIECES[p]
        return remote(wqb.at[g, :, pl.ds(r0, n)], wqb.at[2 + g, :, pl.ds(r0, n)],
                      send_sem.at[1], wqr_sem.at[p], head_peer)

    def wo_load(c):
        return pltpu.make_async_copy(wo_hbm.at[:, pl.ds(c * 256, 256)], wos.at[c], wo_sem.at[c])

    def wo_send(c):
        return remote(wob.at[0, c], wob.at[1, c], send_sem.at[2], wor_sem.at[c], head_peer)

    def kv_load(g, r):
        first = (me if g < 2 else head_peer) * 8 + (g % 2) * 4
        res = slice(None) if r is None else r
        for n, src in enumerate((k_hbm, v_hbm)):
            for h in range(4):
                pltpu.make_async_copy(src.at[:, res, :, first + h, :], kv.at[4 * g + h, n, :, res],
                                      kv_sem.at[4 * g + (r or 0)]).start()

    def kv_wait(g, r):
        wait_all(kv.at[pl.ds(4 * g, 4), :, :, slice(None) if r is None else r], kv_sem.at[4 * g + (r or 0)])

    def wait_all(buf, sem):
        pltpu.make_async_copy(buf, buf, sem).wait()

    def part_send(blk):
        return remote(sendb.at[blk], recvb.at[blk], send_sem.at[3], pr_sem.at[blk], row_peer)

    def add_late(blk):
        c, pair = divmod(blk, 2)
        part_send(blk).wait_recv()
        for s in range(2):
            for j in range(4):
                where = (0, pl.ds(64 * (4 * j + 2 * pair + s), 64), pl.ds(c * 256, 256))
                out_ref[where] = (out_ref[where].astype(F32) + recvb[blk, s, j].astype(F32)).astype(BF16)

    def start(cps):
        for cp in cps:
            cp.start()

    def x_block(rows, n):
        return rows[pl.ds(128 * (n // 2), 128), pl.ds(512 * (n % 2), 512)]

    def x_sums(slot, half):
        for r0 in range(0, 128, 16):
            halves = [half(h, r0).astype(F32) for h in range(2)]
            blocks = [halves[n // 2][:, 512 * (n % 2):512 * (n % 2 + 1)] for n in range(4)]
            for n, j in enumerate(LHS_SUMS):
                val = _operand(LHS[j], lambda b: blocks[b])
                for part in range(2):
                    lhs_ops[X_SUMS + 2 * n + part, pl.ds(128 * slot + r0, 16)] = val[:, 256 * part:256 * (part + 1)]

    def wq_sums(g, half, first, rows):
        for r0 in range(first, first + rows, 32):
            halves = [half(h, pl.ds(r0, 32)) for h in range(2)]
            blocks = [halves[n // 2][:, 256 * (n % 2):256 * (n % 2 + 1)] for n in range(4)]
            for n, j in enumerate(RHS_SUMS):
                wqc[g, n, pl.ds(r0, 32)] = _operand(RHS[j], lambda b: blocks[b])

    def x_ready(p):
        r, j0, n = X_PIECES[p]
        x_load(p).wait()
        xb[r, pl.ds(64 * j0, 64 * n)] = xs[r, pl.ds(j0, n)].reshape(64 * n, 1024).astype(BF16)
        x_send(p).start()
        if j0 + n == 4:
            x_sums(r, lambda h, r0: xs[r, 2 * h + r0 // 64, pl.ds(r0 % 64, 16)])

    def x_recv(p):
        r, j0, n = X_PIECES[p]
        x_send(p).wait_recv()
        if j0 + n == 4:
            x_sums(4 + r, lambda h, r0: xb[4 + r, pl.ds(128 * h + r0, 16)])

    def wq_ready(p):
        g, r0, n = WQ_PIECES[p]
        wq_load(p).wait()
        wqb[g, :, pl.ds(r0, n)] = (wqs[g, :, pl.ds(r0, n)] * Q_SCALE).astype(BF16)
        wq_send(p).start()
        wq_sums(g, lambda h, rows: wqs[g, h, rows] * Q_SCALE, r0, n)

    def wq_recv(p):
        g, r0, n = WQ_PIECES[p]
        wq_send(p).wait_recv()
        wq_sums(2 + g, lambda h, rows: wqb[2 + g, h, rows].astype(F32), r0, n)

    def wo_ready(c):
        wo_load(c).wait()
        wob[0, c] = wos[c].astype(BF16)
        wo_send(c).start()

    events = _plan()[1]
    actions = {"x_ready": x_ready, "wq_ready": wq_ready, "wo_ready": wo_ready,
               "kv_load": lambda key: kv_load(*key),
               "wq_load": lambda p: wq_load(p).start(),
               "wo_load": lambda _: start([wo_load(c) for c in range(4)]),
               "kv_wait": lambda key: kv_wait(*key),
               "x_recv": x_recv,
               "wq_recv": wq_recv,
               "wo_recv": lambda c: wo_send(c).wait_recv()}

    def run_events(i):
        for name, arg in events[i]:
            actions[name](arg)

    def dispatch(index, keys, fn):
        if len(keys) == 1:
            fn(keys[0])
        else:
            mid = len(keys) // 2
            lax.cond(index < keys[mid], lambda: dispatch(index, keys[:mid], fn),
                     lambda: dispatch(index, keys[mid:], fn))

    def attention(slot, g):
        r = slot % 4
        rows = pl.ds(pl.multiple_of(slot * 128, 128), 128)
        scores, ctx = {}, {}

        def qk(h):
            k = kv[4 * g + h, 0, :, r].reshape(256, 128).astype(BF16)
            scores[h] = lax.dot_general(qs[4 * slot + g, :, h * 128:(h + 1) * 128], k, NT_DIMS, preferred_element_type=F32)

        def pv(h):
            s = scores.pop(h)
            p = jnp.exp2(s - jnp.max(s, axis=-1, keepdims=True))
            l = jnp.sum(p, axis=-1, keepdims=True)
            inv = pl.reciprocal(l, approx=True)
            v = kv[4 * g + h, 1, :, r].reshape(256, 128).astype(BF16)
            ctx[h] = _dot(p.astype(BF16), v) * inv

        def emit(h):
            blocks = (ctx[h][:128], ctx[h + 2][:128], ctx[h][128:], ctx[h + 2][128:])
            for j in LHS:
                lhs_ops[7 * g + j - 1, rows, h * 128:(h + 1) * 128] = _operand(LHS[j], lambda b: blocks[b])

        return {"k": qk, "p": pv, "e": emit}

    def projection(slot, g):
        def lhs(j):
            if j not in LHS_SUMS:
                return x_block(xb.at[slot], LHS[j][0])
            rows = pl.ds(pl.multiple_of(slot * 128, 128), 128)
            first = X_SUMS + 2 * LHS_SUMS.index(j)
            return jnp.concatenate([lhs_ops[first, rows, :], lhs_ops[first + 1, rows, :]], axis=1)

        def rhs(j):
            return wqc[g, RHS_SUMS.index(j)] if j in RHS_SUMS else wqb[g, RHS[j][0] // 2, :, pl.ds(256 * (RHS[j][0] % 2), 256)]

        def done(n, val):
            qs[4 * slot + g, pl.ds(128 * (n // 2), 128), pl.ds(256 * (n % 2), 256)] = val.astype(BF16)

        return {"m": _Strassen(lhs, rhs, done).product}

    def run_ops(order, ops):
        for op in order.split():
            ops[op[0]](int(op[1]))

    def o_step(pairs, pair, c, send_blk, *add_blk):
        for n in range(pairs):
            pl.when(add_blk[n] != SPARE)(lambda: part_send(add_blk[n]).wait_recv())

        rows = pl.ds(pl.multiple_of(pair * 256, 256), 256 * pairs)

        def wo_block(n):
            return jnp.concatenate(
                [wob[o, c, pl.ds(q * 512 + (n // 2) * 256, 256), pl.ds((n % 2) * 128, 128)]
                 for o in range(2) for q in range(2)], axis=0)

        def done(n, val):
            half, col = divmod(n, 2)
            cols = pl.ds(pl.multiple_of(c * 256 + col * 128, 128), 128)
            for s in range(2 * pairs):
                for jj in range(2):
                    j = 2 * half + jj
                    piece = val[s * 128 + jj * 64:s * 128 + (jj + 1) * 64]
                    where = (s % 2, j, slice(None), pl.ds(col * 128, 128))
                    out_rows = pl.ds(pl.multiple_of(64 * (4 * j + 2 * (pair % 2) + s), 64), 64)
                    total = piece + recvb[(add_blk[s // 2],) + where].astype(F32)
                    out_ref[0, out_rows, cols] = total.astype(BF16)
                    sendb[(send_blk + s // 2,) + where] = piece.astype(BF16)

        run_ops(O_ORDER, {"m": _Strassen(
            lambda j: jnp.concatenate([lhs_ops[7 * g + j - 1, rows, :] for g in range(4)], axis=1),
            lambda j: _operand(RHS[j], wo_block), done).product})

        @pl.when(send_blk != SPARE)
        def _():
            for n in range(pairs):
                part_send(send_blk + n).start()

    barrier = pltpu.get_barrier_semaphore()
    for peer in (row_peer, head_peer):
        pl.semaphore_signal(barrier, inc=1, device_id=(peer,), device_id_type=pl.DeviceIdType.MESH)
    start([wq_load(0), x_load(0), x_load(1), wq_load(1), wq_load(2), wq_load(3),
           x_load(2), x_load(3), x_load(4), wq_load(4), wq_load(5)])
    kv_load(0, 0)
    recvb[SPARE] = jnp.zeros(recvb.shape[1:], BF16)
    pl.semaphore_wait(barrier, 2)
    wq_ready(0)
    x_ready(0)
    x_ready(1)
    for p in range(1, 4):
        wq_ready(p)
    kv_load(0, 1)

    def step(i, carry):
        has_events, body, *arg = (tab[TABLE_WIDTH * i + n] for n in range(TABLE_WIDTH))
        pl.when(has_events != 0)(lambda: dispatch(i, sorted(events), run_events))

        def run(code):
            kind, n = BODIES[code]
            if kind == "P":
                run_ops(P_ORDER, projection(*arg[:2]))
            elif kind == "A":
                heads = [attention(*arg[2 * u:2 * u + 2]) for u in range(n)]
                for op in A_ORDER.split():
                    for ops in heads:
                        ops[op[0]](int(op[1]))
            elif kind == "Q":
                for u in range(n):
                    run_ops(QA_ORDER, {**attention(*arg[4 * u:4 * u + 2]), **projection(*arg[4 * u + 2:4 * u + 4])})
            else:
                o_step(n, *arg[:3 + n])

        dispatch(body, list(range(len(BODIES))), run)
        return carry

    lax.fori_loop(0, len(SCHEDULE), step, None)

    for pair, c in LATE:
        add_late(2 * c + pair)
    for n, sent in enumerate((xb.at[pl.ds(0, 4)], wqb.at[pl.ds(0, 2)], wob.at[0], sendb.at[pl.ds(0, 8)])):
        wait_all(sent, send_sem.at[n])


def pallas_dist_sparse_attn_strided_qseq_b1_sq1024_skv1024_hq8_dh128_kernel(x, Wq, K_ext, V_ext, Wo):
    dma = pltpu.SemaphoreType.DMA
    hbm = pl.BlockSpec(memory_space=pltpu.HBM)
    out = pl.pallas_call(
        _body,
        out_shape=pltpu.VMEM((1, 1024, 1024), BF16),
        in_specs=[pl.BlockSpec(memory_space=pltpu.SMEM), hbm, hbm, hbm, hbm, hbm],
        out_specs=pl.BlockSpec(memory_space=pltpu.VMEM),
        scratch_shapes=[
            pltpu.VMEM((4, 4, 64, 1024), F32),
            pltpu.VMEM((8, 256, 1024), BF16),
            pltpu.VMEM((2, 2, 512, 512), F32),
            pltpu.VMEM((4, 2, 512, 512), BF16),
            pltpu.VMEM((4, 5, 512, 256), BF16),
            pltpu.VMEM((4, 1024, 256), F32),
            pltpu.VMEM((2, 4, 1024, 256), BF16),
            pltpu.VMEM((16, 2, 4, 4, 64, 128), F32),
            pltpu.VMEM((32, 256, 512), BF16),
            pltpu.VMEM((X_SUMS + 10, 1024, 256), BF16),
            pltpu.VMEM((10, 2, 4, 64, 256), BF16),
            pltpu.VMEM((9, 2, 4, 64, 256), BF16),
            dma((len(X_PIECES),)), dma((len(WQ_PIECES),)), dma((4,)), dma((16,)),
            dma((4,)),
            dma((len(X_PIECES),)), dma((len(WQ_PIECES),)), dma((4,)), dma((8,)),
        ],
        compiler_params=pltpu.CompilerParams(collective_id=0, vmem_limit_bytes=100 * 1024 * 1024),
    )(
        _plan()[0],
        x.reshape(4, 4, 64, 1024),
        Wq.reshape(2, 512, 1024),
        K_ext.reshape(4, 4, 64, 32, 128),
        V_ext.reshape(4, 4, 64, 32, 128),
        Wo,
    )
    return out
```
